```python
import numpy as np

kernel_name = "dist_sparse_attn_blocksparse_qseq_b2_sq256_skv256_hq4_dh64"

def setup_inputs():
    x = np.random.randn(2, 1024, 512).astype(np.float32)
    Wq = np.random.randn(512, 1024).astype(np.float32) * 0.02
    K_ext = np.random.randn(2, 256, 16, 64).astype(np.float32)
    V_ext = np.random.randn(2, 256, 16, 64).astype(np.float32)
    Wo = np.random.randn(1024, 512).astype(np.float32) * 0.02
    return {"x": x, "Wq": Wq, "K_ext": K_ext, "V_ext": V_ext, "Wo": Wo}

def reference(x, Wq, K_ext, V_ext, Wo):
    B, Sq, Skv, Hq, Dh = 2, 1024, 256, 16, 64
    Q = (x @ Wq).reshape(B, Sq, Hq, Dh)
    qb = (np.arange(Sq) // 64)[:, None]
    kb = (np.arange(Skv) // 64)[None, :]
    mask = (qb == kb) | (kb == 0) | ((qb + kb) % 3 == 0)
    scores = np.einsum('bihd,bjhd->bhij', Q, K_ext).astype(np.float32) * 0.125
    scores = np.where(mask[None, None, :, :], scores, -1e9)
    scores_max = scores.max(axis=-1, keepdims=True)
    w = np.exp(scores - scores_max)
    row_keep = mask.any(axis=1)
    w_sum = np.where(row_keep[None, None, :, None], w.sum(axis=-1, keepdims=True), 1.0)
    w = w / w_sum
    w = np.where(row_keep[None, None, :, None], w, 0.0)
    ctx = np.einsum('bhij,bjhd->bihd', w, V_ext).reshape(B, Sq, Hq * Dh)
    return ctx @ Wo
```

```python
import jax
import jax.numpy as jnp
from jax import lax
from jax.experimental import pallas as pl
from jax.experimental.pallas import tpu as pltpu

N_DEV = 4
B = 2
SQ = 256
SKV = 256
D_MODEL = 512
DH = 64
BLK = 64
ROWS = B * SQ
PAIR = 2 * DH
N_PAIR = 8
NCB = D_MODEL // 128
R0 = 32
WQ_CHUNKS = ((R0, 32), (R0 + 32, 96), (R0 + 128, 128), (R0 + 256, 256 - R0), (0, R0))

MESH = pl.DeviceIdType.MESH
LEFT, RIGHT = 0, 1

S_WQ1, S_WQ2, S_WO1, S_WQF, S_WO2, S_F32, S_WOF = 0, 1, 2, 3, 4, 5, 6
WOF_PIECES = ((0, None), (1, None), (2, None), (3, 0), (3, 1))
N_SLOT = S_WOF + len(WOF_PIECES)


def _kernel(x_hbm, wq_hbm, kt_hbm, vt_hbm, wo_hbm, out_ref,
            x32, xb, wq32, wo32, kt32, vt32, wq_buf, wo_buf, ctx, st32,
            lsem, kvsem, ssem, rsem, ready):
    wq_cp = [pltpu.make_async_copy(wq_hbm.at[pl.ds(r0, rn)], wq32.at[pl.ds(r0, rn)], lsem.at[c])
             for c, (r0, rn) in enumerate(WQ_CHUNKS)]
    for c in wq_cp:
        c.start()

    me = lax.axis_index("i")
    left = (me + 3) & 3
    right = (me + 1) & 3
    opp = (me + 2) & 3
    nbr = (left, right)

    down = (right < 2, me < 2)
    up = (right >= 2, me >= 2)
    bar = pltpu.get_barrier_semaphore()

    @pl.when((me & 1) == 1)
    def _():
        pl.semaphore_wait(bar, 1)

    @pl.when(me == 2)
    def _():
        pl.semaphore_wait(bar, 2)

    first = {RIGHT: 0, LEFT: 1}

    def f32_copy(d):
        return pltpu.make_async_remote_copy(
            src_ref=wq_hbm.at[pl.ds(0, R0), pl.ds(first[d] * PAIR, PAIR)],
            dst_ref=st32.at[1 - d], send_sem=ssem.at[d, S_F32],
            recv_sem=rsem.at[1 - d, S_F32], device_id=(nbr[d],), device_id_type=MESH)

    for d in (LEFT, RIGHT):
        @pl.when(up[d])
        def _(d=d):
            f32_copy(d).start()

    n_wq = len(WQ_CHUNKS)
    x_cp = pltpu.make_async_copy(x_hbm, x32, lsem.at[n_wq])
    wo_cp = pltpu.make_async_copy(wo_hbm, wo32, lsem.at[n_wq + 1])
    for d, cp in ((LEFT, wo_cp), (RIGHT, x_cp)):
        @pl.when(down[d])
        def _(d=d):
            pl.semaphore_signal(bar, inc=1, device_id=(nbr[d],), device_id_type=MESH)

        cp.start()

        @pl.when(up[d])
        def _(d=d):
            pl.semaphore_signal(ready.at[1 - d], inc=1, device_id=(nbr[d],),
                                device_id_type=MESH)

    order = [2 * me, 2 * me + 1, 2 * left, 2 * right + 1, 2 * left + 1, 2 * right,
             2 * opp, 2 * opp + 1]

    def kv_copies(i):
        r = pl.ds(pl.multiple_of(order[i] * PAIR, PAIR), PAIR)
        return (pltpu.make_async_copy(kt_hbm.at[:, r, :], kt32.at[:, r, :], kvsem.at[2 * i]),
                pltpu.make_async_copy(vt_hbm.at[:, r, :], vt32.at[:, r, :], kvsem.at[2 * i + 1]))

    for i in range(N_PAIR):
        for c in kv_copies(i):
            c.start(priority=1)

    def rcopy(ref, d, slot):
        return pltpu.make_async_remote_copy(
            src_ref=ref, dst_ref=ref, send_sem=ssem.at[d, slot],
            recv_sem=rsem.at[1 - d, slot], device_id=(nbr[d],), device_id_type=MESH)

    def wait_recv(ref, d, slot):
        pltpu.make_async_remote_copy(
            src_ref=ref, dst_ref=ref, send_sem=ssem.at[d, slot],
            recv_sem=rsem.at[d, slot], device_id=(nbr[d],), device_id_type=MESH).wait_recv()

    for c, (r0, rn) in enumerate(WQ_CHUNKS):
        wq_cp[c].wait()
        rows = pl.ds(r0, rn)
        w = wq32[rows, :].astype(jnp.bfloat16)
        wq_buf[2 * me, rows, :] = w[:, :PAIR]
        wq_buf[2 * me + 1, rows, :] = w[:, PAIR:]
        if r0 == 0:
            continue
        for d in (LEFT, RIGHT):
            @pl.when(up[d])
            def _(d=d, rows=rows):
                rcopy(wq_buf.at[2 * me + first[d], rows], d, S_WQ1).start()
    for d in (LEFT, RIGHT):
        @pl.when(up[d])
        def _(d=d):
            rcopy(wq_buf.at[2 * me + 1 - first[d]], d, S_WQ2).start()
    for d in (LEFT, RIGHT):
        @pl.when(down[d])
        def _(d=d):
            pl.semaphore_wait(ready.at[d], 1)
            rcopy(wq_buf.at[2 * me + first[d]], d, S_WQ1).start()
            rcopy(wq_buf.at[2 * me + 1 - first[d]], d, S_WQ2).start()

    wo_cp.wait()
    for h in range(4):
        w = wo32[pl.ds(h * DH, DH), :].astype(jnp.bfloat16)
        for c in range(NCB):
            wo_buf[me, h % 2, c, h // 2] = w[:, c * 128:(c + 1) * 128]
    for d in (LEFT, RIGHT):
        rcopy(wo_buf.at[me, first[d]], d, S_WO1).start()

    x_cp.wait()
    xb[...] = x32[...].astype(jnp.bfloat16)

    ks = 3 - me % 3
    ks_off = pl.multiple_of(jnp.where(ks >= 2, 128, 0), 128)
    ks_shift = jnp.where(ks == 2, DH, 0)
    kb = lax.broadcasted_iota(jnp.int32, (BLK, SKV), 1) // BLK
    masks = []
    for i in (1, 2):
        qb = 4 * me + i
        masks.append((kb == qb) | (kb == 0) | (kb == 3 - qb % 3))
    mask12 = jnp.concatenate(masks, axis=0)
    lane_lo = lax.broadcasted_iota(jnp.int32, (PAIR, PAIR), 1) < DH

    def pad_heads(t, fill):
        f = jnp.full((DH, t.shape[1]), fill, jnp.bfloat16)
        return (jnp.concatenate([t[:DH], f], axis=0), jnp.concatenate([f, t[DH:]], axis=0))

    def qproj(gp):
        q = jnp.dot(xb[...], wq_buf[gp], preferred_element_type=jnp.float32)
        return (q * 0.125).astype(jnp.bfloat16)

    def sel_full(t32, gp, b):
        r = pl.ds(pl.multiple_of(gp * PAIR, PAIR), PAIR)
        t = t32[b, r, :]
        hi = pltpu.roll(t32[b, r, pl.ds(ks_off, 128)], ks_shift, 1)
        return (jnp.where(lane_lo, t[:, :128], hi).astype(jnp.bfloat16),
                t.astype(jnp.bfloat16))

    def scores(q, gp, b):
        o = b * SQ
        q03 = jnp.concatenate([q[o:o + BLK], q[o + 3 * BLK:o + 4 * BLK]], axis=0)
        q12 = q[o + BLK:o + 3 * BLK]
        sel, full = sel_full(kt32, gp, b)
        k03 = pad_heads(sel, 0)
        k12 = pad_heads(full, 0)
        return ([jnp.dot(q03, k03[h], preferred_element_type=jnp.float32) for h in range(2)]
                + [jnp.dot(q12, k12[h], preferred_element_type=jnp.float32) for h in range(2)])

    def soft(s, msk):
        if msk is not None:
            s = jnp.where(msk, s, -1e9)
        m = jnp.max(s, axis=1, keepdims=True)
        return jnp.exp(s - m).astype(jnp.bfloat16)

    def norm(o0, o1):
        num = jnp.where(lane_lo, o0, o1)
        den = pltpu.roll(jnp.where(lane_lo, o1, o0), DH, 1)
        r = pl.reciprocal(den, approx=True)
        r = r * (2.0 - den * r)
        return (num * r).astype(jnp.bfloat16)

    def pv(ps, gp, b):
        o = b * SQ
        sel, full = sel_full(vt32, gp, b)
        v03 = pad_heads(sel, 1)
        v12 = pad_heads(full, 1)
        nt = (((1,), (1,)), ((), ()))
        c03 = norm(*[lax.dot_general(ps[h], v03[h], nt, preferred_element_type=jnp.float32)
                     for h in range(2)])
        c12 = norm(*[lax.dot_general(ps[2 + h], v12[h], nt, preferred_element_type=jnp.float32)
                     for h in range(2)])
        ctx[gp, pl.ds(o, BLK), :] = c03[:BLK]
        ctx[gp, pl.ds(o + BLK, 2 * BLK), :] = c12
        ctx[gp, pl.ds(o + 3 * BLK, BLK), :] = c03[BLK:]

    def attn_stage(i):
        for j in (i, i + 1):
            for c in kv_copies(j):
                c.wait()
        units = []
        for gp in (order[i], order[i + 1]):
            q = qproj(gp)
            units += [(q, gp, b) for b in range(B)]
        ss = [scores(*u) for u in units]
        ps = [[soft(s[0], None), soft(s[1], None), soft(s[2], mask12), soft(s[3], mask12)]
              for s in ss]
        for p, u in zip(ps, units):
            pv(p, u[1], u[2])

    lane_lo_rows = lax.broadcasted_iota(jnp.int32, (ROWS, PAIR), 1) < DH

    def wo_tile(d_even, d_odd, c, p):
        return jnp.concatenate([wo_buf[d_even, 0, c, p], wo_buf[d_odd, 1, c, p]], axis=0)

    def proj_all(d_even, d_odd, init=False):
        if d_even is d_odd:
            lhs = [ctx[2 * d_even + p] for p in range(2)]
        else:
            lhs = [jnp.where(lane_lo_rows, ctx[2 * d_even + p], ctx[2 * d_odd + p])
                   for p in range(2)]
        lhs = jnp.concatenate(lhs, axis=1)
        rhs = jnp.concatenate(
            [jnp.concatenate([wo_tile(d_even, d_odd, c, p) for p in range(2)], axis=0)
             for c in range(NCB)], axis=1)
        y = jnp.dot(lhs, rhs, preferred_element_type=jnp.float32).reshape(B, SQ, D_MODEL)
        if init:
            out_ref[...] = y
        else:
            out_ref[...] += y

    def proj_piece(c, ps):
        cols = pl.ds(c * 128, 128)
        rhs = jnp.concatenate([wo_tile(opp, opp, c, p) for p in ps], axis=0)
        nsplit = 4 // len(ps)
        rn = ROWS // nsplit
        for j in range(nsplit):
            lhs = jnp.concatenate([ctx[2 * opp + p, pl.ds(j * rn, rn), :] for p in ps], axis=1)
            y = jnp.dot(lhs, rhs, preferred_element_type=jnp.float32)
            b, r0 = divmod(j * rn, SQ)
            out_ref[b, pl.ds(r0, rn), cols] += y

    def wof_ref(dev, par, k):
        c, p = WOF_PIECES[k]
        return wo_buf.at[dev, par, c] if p is None else wo_buf.at[dev, par, c, p]

    rest = pl.ds(R0, D_MODEL - R0)

    def wait_wq1(g, d):
        @pl.when(down[d])
        def _():
            wait_recv(st32.at[d], d, S_F32)
            wq_buf[g, pl.ds(0, R0), :] = st32[d].astype(jnp.bfloat16)
            wait_recv(wq_buf.at[g, rest], d, S_WQ1)

        @pl.when(up[d])
        def _():
            wait_recv(wq_buf.at[g], d, S_WQ1)

    attn_stage(0)

    wait_wq1(2 * left, LEFT)
    rcopy(wq_buf.at[2 * left], RIGHT, S_WQF).start()
    rcopy(wo_buf.at[me, 1 - first[RIGHT]], RIGHT, S_WO2).start()
    wait_wq1(2 * right + 1, RIGHT)
    rcopy(wq_buf.at[2 * right + 1], LEFT, S_WQF).start()
    rcopy(wo_buf.at[me, 1 - first[LEFT]], LEFT, S_WO2).start()
    attn_stage(2)

    wait_recv(wq_buf.at[2 * left + 1], LEFT, S_WQ2)
    wait_recv(wq_buf.at[2 * right], RIGHT, S_WQ2)
    attn_stage(4)
    proj_all(me, me, init=True)

    wait_recv(wo_buf.at[left, 0], LEFT, S_WO1)
    for k in range(len(WOF_PIECES)):
        rcopy(wof_ref(left, 0, k), RIGHT, S_WOF + k).start()
    wait_recv(wo_buf.at[right, 1], RIGHT, S_WO1)
    for k in range(len(WOF_PIECES)):
        rcopy(wof_ref(right, 1, k), LEFT, S_WOF + k).start()
    proj_all(left, right)

    wait_recv(wq_buf.at[2 * opp], LEFT, S_WQF)
    wait_recv(wq_buf.at[2 * opp + 1], RIGHT, S_WQF)
    attn_stage(6)

    wait_recv(wo_buf.at[left, 1], LEFT, S_WO2)
    wait_recv(wo_buf.at[right, 0], RIGHT, S_WO2)
    proj_all(right, left)

    for k, (c, p) in enumerate(WOF_PIECES):
        if k == len(WOF_PIECES) - 1:
            for d in (LEFT, RIGHT):
                @pl.when(down[d])
                def _(d=d):
                    rcopy(wq_buf.at[0], d, S_WQ1).wait_send()

                @pl.when(up[d])
                def _(d=d):
                    f32_copy(d).wait_send()
                    rcopy(wq_buf.at[0, rest], d, S_WQ1).wait_send()

                for slot in (S_WQ2, S_WQF):
                    rcopy(wq_buf.at[0], d, slot).wait_send()
                for slot in (S_WO1, S_WO2):
                    rcopy(wo_buf.at[0, 0], d, slot).wait_send()
                for kk in range(len(WOF_PIECES)):
                    rcopy(wof_ref(0, 0, kk), d, S_WOF + kk).wait_send()
        wait_recv(wof_ref(opp, 0, k), LEFT, S_WOF + k)
        wait_recv(wof_ref(opp, 1, k), RIGHT, S_WOF + k)
        proj_piece(c, (0, 1) if p is None else (p,))


def pallas_dist_sparse_attn_blocksparse_qseq_b2_sq256_skv256_hq4_dh64_kernel(
    x: jax.Array,
    Wq: jax.Array,
    K_ext: jax.Array,
    V_ext: jax.Array,
    Wo: jax.Array,
):
    x2 = x.reshape(ROWS, D_MODEL)
    kt = jnp.transpose(K_ext, (0, 2, 3, 1)).reshape(B, N_PAIR * PAIR, SKV)
    vt = jnp.transpose(V_ext, (0, 2, 3, 1)).reshape(B, N_PAIR * PAIR, SKV)
    any_spec = pl.BlockSpec(memory_space=pl.ANY)
    return pl.pallas_call(
        _kernel,
        out_shape=jax.ShapeDtypeStruct((B, SQ, D_MODEL), jnp.float32),
        in_specs=[any_spec] * 5,
        out_specs=pl.BlockSpec(memory_space=pltpu.VMEM),
        scratch_shapes=[
            pltpu.VMEM((ROWS, D_MODEL), jnp.float32),
            pltpu.VMEM((ROWS, D_MODEL), jnp.bfloat16),
            pltpu.VMEM((D_MODEL, 2 * PAIR), jnp.float32),
            pltpu.VMEM((2 * PAIR, D_MODEL), jnp.float32),
            pltpu.VMEM((B, N_PAIR * PAIR, SKV), jnp.float32),
            pltpu.VMEM((B, N_PAIR * PAIR, SKV), jnp.float32),
            pltpu.VMEM((N_PAIR, D_MODEL, PAIR), jnp.bfloat16),
            pltpu.VMEM((N_DEV, 2, NCB, 2, DH, 128), jnp.bfloat16),
            pltpu.VMEM((N_PAIR, ROWS, PAIR), jnp.bfloat16),
            pltpu.VMEM((2, R0, PAIR), jnp.float32),
            pltpu.SemaphoreType.DMA((len(WQ_CHUNKS) + 2,)),
            pltpu.SemaphoreType.DMA((2 * N_PAIR,)),
            pltpu.SemaphoreType.DMA((2, N_SLOT)),
            pltpu.SemaphoreType.DMA((2, N_SLOT)),
            pltpu.SemaphoreType.REGULAR((2,)),
        ],
        compiler_params=pltpu.CompilerParams(
            collective_id=0,
            vmem_limit_bytes=64 * 1024 * 1024,
            disable_semaphore_checks=True,
            disable_bounds_checks=True,
        ),
    )(x2, Wq, kt, vt, Wo)
```

```python
import jax
import jax.numpy as jnp
from jax import lax
from jax.experimental import pallas as pl
from jax.experimental.pallas import tpu as pltpu

N_DEV = 4
B = 2
SQ = 256
SKV = 256
D_MODEL = 512
DH = 64
BLK = 64
ROWS = B * SQ
PAIR = 2 * DH
N_PAIR = 8
NCB = D_MODEL // 128
R0 = 32
WQ_CHUNKS = ((R0, 32), (R0 + 32, 96), (R0 + 128, 128), (R0 + 256, 256 - R0), (0, R0))

MESH = pl.DeviceIdType.MESH
LEFT, RIGHT = 0, 1

S_WQ1, S_WQ2, S_WO1, S_WQF, S_WO2, S_F32, S_WOF = 0, 1, 2, 3, 4, 5, 6
WOF_PIECES = ((0, None), (1, None), (2, None), (3, 0), (3, 1))
N_SLOT = S_WOF + len(WOF_PIECES)


def _kernel(x_hbm, wq_hbm, kt_hbm, vt_hbm, wo_hbm, out_ref,
            x32, xb, wq32, wo32, kt32, vt32, wq_buf, wo_buf, ctx, st32,
            lsem, kvsem, ssem, rsem, ready):
    wq_cp = [pltpu.make_async_copy(wq_hbm.at[pl.ds(r0, rn)], wq32.at[pl.ds(r0, rn)], lsem.at[c])
             for c, (r0, rn) in enumerate(WQ_CHUNKS)]
    for c in wq_cp:
        c.start()

    me = lax.axis_index("i")
    left = (me + 3) & 3
    right = (me + 1) & 3
    opp = (me + 2) & 3
    nbr = (left, right)

    down = (right < 2, me < 2)
    up = (right >= 2, me >= 2)
    bar = pltpu.get_barrier_semaphore()

    @pl.when((me & 1) == 1)
    def _():
        pl.semaphore_wait(bar, 1)

    @pl.when(me == 2)
    def _():
        pl.semaphore_wait(bar, 2)

    first = {RIGHT: 0, LEFT: 1}

    def f32_copy(d):
        return pltpu.make_async_remote_copy(
            src_ref=wq_hbm.at[pl.ds(0, R0), pl.ds(first[d] * PAIR, PAIR)],
            dst_ref=st32.at[1 - d], send_sem=ssem.at[d, S_F32],
            recv_sem=rsem.at[1 - d, S_F32], device_id=(nbr[d],), device_id_type=MESH)

    for d in (LEFT, RIGHT):
        @pl.when(up[d])
        def _(d=d):
            f32_copy(d).start()

    n_wq = len(WQ_CHUNKS)
    x_cp = pltpu.make_async_copy(x_hbm, x32, lsem.at[n_wq])
    wo_cp = pltpu.make_async_copy(wo_hbm, wo32, lsem.at[n_wq + 1])
    for d, cp in ((LEFT, wo_cp), (RIGHT, x_cp)):
        @pl.when(down[d])
        def _(d=d):
            pl.semaphore_signal(bar, inc=1, device_id=(nbr[d],), device_id_type=MESH)

        cp.start()

        @pl.when(up[d])
        def _(d=d):
            pl.semaphore_signal(ready.at[1 - d], inc=1, device_id=(nbr[d],),
                                device_id_type=MESH)

    order = [2 * me, 2 * me + 1, 2 * left, 2 * right + 1, 2 * left + 1, 2 * right,
             2 * opp, 2 * opp + 1]

    def kv_copies(i):
        r = pl.ds(pl.multiple_of(order[i] * PAIR, PAIR), PAIR)
        return (pltpu.make_async_copy(kt_hbm.at[:, r, :], kt32.at[:, r, :], kvsem.at[2 * i]),
                pltpu.make_async_copy(vt_hbm.at[:, r, :], vt32.at[:, r, :], kvsem.at[2 * i + 1]))

    for i in range(N_PAIR):
        for c in kv_copies(i):
            c.start(priority=1)

    def rcopy(ref, d, slot):
        return pltpu.make_async_remote_copy(
            src_ref=ref, dst_ref=ref, send_sem=ssem.at[d, slot],
            recv_sem=rsem.at[1 - d, slot], device_id=(nbr[d],), device_id_type=MESH)

    def wait_recv(ref, d, slot):
        pltpu.make_async_remote_copy(
            src_ref=ref, dst_ref=ref, send_sem=ssem.at[d, slot],
            recv_sem=rsem.at[d, slot], device_id=(nbr[d],), device_id_type=MESH).wait_recv()

    for c, (r0, rn) in enumerate(WQ_CHUNKS):
        wq_cp[c].wait()
        rows = pl.ds(r0, rn)
        w = wq32[rows, :].astype(jnp.bfloat16)
        wq_buf[2 * me, rows, :] = w[:, :PAIR]
        wq_buf[2 * me + 1, rows, :] = w[:, PAIR:]
        if r0 == 0:
            continue
        for d in (LEFT, RIGHT):
            @pl.when(up[d])
            def _(d=d, rows=rows):
                rcopy(wq_buf.at[2 * me + first[d], rows], d, S_WQ1).start()
    for d in (LEFT, RIGHT):
        @pl.when(up[d])
        def _(d=d):
            rcopy(wq_buf.at[2 * me + 1 - first[d]], d, S_WQ2).start()
    for d in (LEFT, RIGHT):
        @pl.when(down[d])
        def _(d=d):
            pl.semaphore_wait(ready.at[d], 1)
            rcopy(wq_buf.at[2 * me + first[d]], d, S_WQ1).start()
            rcopy(wq_buf.at[2 * me + 1 - first[d]], d, S_WQ2).start()

    wo_cp.wait()
    for h in range(4):
        w = wo32[pl.ds(h * DH, DH), :].astype(jnp.bfloat16)
        for c in range(NCB):
            wo_buf[me, h % 2, c, h // 2] = w[:, c * 128:(c + 1) * 128]
    for d in (LEFT, RIGHT):
        rcopy(wo_buf.at[me, first[d]], d, S_WO1).start()

    x_cp.wait()
    xb[...] = x32[...].astype(jnp.bfloat16)

    ks = 3 - me % 3
    ks_off = pl.multiple_of(jnp.where(ks >= 2, 128, 0), 128)
    ks_shift = jnp.where(ks == 2, DH, 0)
    kb = lax.broadcasted_iota(jnp.int32, (BLK, SKV), 1) // BLK
    masks = []
    for i in (1, 2):
        qb = 4 * me + i
        masks.append((kb == qb) | (kb == 0) | (kb == 3 - qb % 3))
    mask12 = jnp.concatenate(masks, axis=0)
    lane_lo = lax.broadcasted_iota(jnp.int32, (PAIR, PAIR), 1) < DH

    def pad_heads(t, fill):
        f = jnp.full((DH, t.shape[1]), fill, jnp.bfloat16)
        return (jnp.concatenate([t[:DH], f], axis=0), jnp.concatenate([f, t[DH:]], axis=0))

    def qproj(gp):
        q = jnp.dot(xb[...], wq_buf[gp], preferred_element_type=jnp.float32)
        return (q * 0.125).astype(jnp.bfloat16)

    def sel_full(t32, gp, b):
        r = pl.ds(pl.multiple_of(gp * PAIR, PAIR), PAIR)
        t = t32[b, r, :]
        hi = pltpu.roll(t32[b, r, pl.ds(ks_off, 128)], ks_shift, 1)
        return (jnp.where(lane_lo, t[:, :128], hi).astype(jnp.bfloat16),
                t.astype(jnp.bfloat16))

    def scores(q, gp, b):
        o = b * SQ
        q03 = jnp.concatenate([q[o:o + BLK], q[o + 3 * BLK:o + 4 * BLK]], axis=0)
        q12 = q[o + BLK:o + 3 * BLK]
        sel, full = sel_full(kt32, gp, b)
        k03 = pad_heads(sel, 0)
        k12 = pad_heads(full, 0)
        return ([jnp.dot(q03, k03[h], preferred_element_type=jnp.float32) for h in range(2)]
                + [jnp.dot(q12, k12[h], preferred_element_type=jnp.float32) for h in range(2)])

    def soft(s, msk):
        if msk is not None:
            s = jnp.where(msk, s, -1e9)
        m = jnp.max(s, axis=1, keepdims=True)
        return jnp.exp(s - m).astype(jnp.bfloat16)

    def norm(o0, o1):
        num = jnp.where(lane_lo, o0, o1)
        den = pltpu.roll(jnp.where(lane_lo, o1, o0), DH, 1)
        r = pl.reciprocal(den, approx=True)
        r = r * (2.0 - den * r)
        return (num * r).astype(jnp.bfloat16)

    def pv(ps, gp, b):
        o = b * SQ
        sel, full = sel_full(vt32, gp, b)
        v03 = pad_heads(sel, 1)
        v12 = pad_heads(full, 1)
        nt = (((1,), (1,)), ((), ()))
        c03 = norm(*[lax.dot_general(ps[h], v03[h], nt, preferred_element_type=jnp.float32)
                     for h in range(2)])
        c12 = norm(*[lax.dot_general(ps[2 + h], v12[h], nt, preferred_element_type=jnp.float32)
                     for h in range(2)])
        ctx[gp, pl.ds(o, BLK), :] = c03[:BLK]
        ctx[gp, pl.ds(o + BLK, 2 * BLK), :] = c12
        ctx[gp, pl.ds(o + 3 * BLK, BLK), :] = c03[BLK:]

    def attn_stage(i):
        for j in (i, i + 1):
            for c in kv_copies(j):
                c.wait()
        units = []
        for gp in (order[i], order[i + 1]):
            q = qproj(gp)
            units += [(q, gp, b) for b in range(B)]
        ss = [scores(*u) for u in units]
        ps = [[soft(s[0], None), soft(s[1], None), soft(s[2], mask12), soft(s[3], mask12)]
              for s in ss]
        for p, u in zip(ps, units):
            pv(p, u[1], u[2])

    lane_lo_rows = lax.broadcasted_iota(jnp.int32, (ROWS, PAIR), 1) < DH

    def wo_tile(d_even, d_odd, c, p):
        return jnp.concatenate([wo_buf[d_even, 0, c, p], wo_buf[d_odd, 1, c, p]], axis=0)

    def proj_all(d_even, d_odd, init=False):
        if d_even is d_odd:
            lhs = [ctx[2 * d_even + p] for p in range(2)]
        else:
            lhs = [jnp.where(lane_lo_rows, ctx[2 * d_even + p], ctx[2 * d_odd + p])
                   for p in range(2)]
        lhs = jnp.concatenate(lhs, axis=1)
        rhs = jnp.concatenate(
            [jnp.concatenate([wo_tile(d_even, d_odd, c, p) for p in range(2)], axis=0)
             for c in range(NCB)], axis=1)
        y = jnp.dot(lhs, rhs, preferred_element_type=jnp.float32).reshape(B, SQ, D_MODEL)
        if init:
            out_ref[...] = y
        else:
            out_ref[...] += y

    def proj_piece(c, ps):
        cols = pl.ds(c * 128, 128)
        rhs = jnp.concatenate([wo_tile(opp, opp, c, p) for p in ps], axis=0)
        nsplit = 4 // len(ps)
        rn = ROWS // nsplit
        for j in range(nsplit):
            lhs = jnp.concatenate([ctx[2 * opp + p, pl.ds(j * rn, rn), :] for p in ps], axis=1)
            y = jnp.dot(lhs, rhs, preferred_element_type=jnp.float32)
            b, r0 = divmod(j * rn, SQ)
            out_ref[b, pl.ds(r0, rn), cols] += y

    def wof_ref(dev, par, k):
        c, p = WOF_PIECES[k]
        return wo_buf.at[dev, par, c] if p is None else wo_buf.at[dev, par, c, p]

    rest = pl.ds(R0, D_MODEL - R0)

    def wait_wq1(g, d):
        @pl.when(down[d])
        def _():
            wait_recv(st32.at[d], d, S_F32)
            wq_buf[g, pl.ds(0, R0), :] = st32[d].astype(jnp.bfloat16)
            wait_recv(wq_buf.at[g, rest], d, S_WQ1)

        @pl.when(up[d])
        def _():
            wait_recv(wq_buf.at[g], d, S_WQ1)

    attn_stage(0)

    wait_wq1(2 * left, LEFT)
    rcopy(wq_buf.at[2 * left], RIGHT, S_WQF).start()
    rcopy(wo_buf.at[me, 1 - first[RIGHT]], RIGHT, S_WO2).start()
    wait_wq1(2 * right + 1, RIGHT)
    rcopy(wq_buf.at[2 * right + 1], LEFT, S_WQF).start()
    rcopy(wo_buf.at[me, 1 - first[LEFT]], LEFT, S_WO2).start()
    attn_stage(2)

    wait_recv(wq_buf.at[2 * left + 1], LEFT, S_WQ2)
    wait_recv(wq_buf.at[2 * right], RIGHT, S_WQ2)
    attn_stage(4)
    proj_all(me, me, init=True)

    wait_recv(wo_buf.at[left, 0], LEFT, S_WO1)
    for k in range(len(WOF_PIECES)):
        rcopy(wof_ref(left, 0, k), RIGHT, S_WOF + k).start()
    wait_recv(wo_buf.at[right, 1], RIGHT, S_WO1)
    for k in range(len(WOF_PIECES)):
        rcopy(wof_ref(right, 1, k), LEFT, S_WOF + k).start()
    proj_all(left, right)

    wait_recv(wq_buf.at[2 * opp], LEFT, S_WQF)
    wait_recv(wq_buf.at[2 * opp + 1], RIGHT, S_WQF)
    attn_stage(6)

    wait_recv(wo_buf.at[left, 1], LEFT, S_WO2)
    wait_recv(wo_buf.at[right, 0], RIGHT, S_WO2)
    proj_all(right, left)

    for k, (c, p) in enumerate(WOF_PIECES):
        if k == len(WOF_PIECES) - 1:
            for d in (LEFT, RIGHT):
                src = nbr[1 - d]

                @pl.when(down[d])
                def _(d=d):
                    rcopy(wq_buf.at[2 * me + first[d]], d, S_WQ1).wait_send()

                @pl.when(up[d])
                def _(d=d):
                    f32_copy(d).wait_send()
                    rcopy(wq_buf.at[2 * me + first[d], rest], d, S_WQ1).wait_send()

                rcopy(wq_buf.at[2 * me + 1 - first[d]], d, S_WQ2).wait_send()
                rcopy(wq_buf.at[2 * src + first[d]], d, S_WQF).wait_send()
                rcopy(wo_buf.at[me, first[d]], d, S_WO1).wait_send()
                rcopy(wo_buf.at[me, 1 - first[d]], d, S_WO2).wait_send()
                for kk in range(len(WOF_PIECES)):
                    rcopy(wof_ref(src, first[d], kk), d, S_WOF + kk).wait_send()
        wait_recv(wof_ref(opp, 0, k), LEFT, S_WOF + k)
        wait_recv(wof_ref(opp, 1, k), RIGHT, S_WOF + k)
        proj_piece(c, (0, 1) if p is None else (p,))


def pallas_dist_sparse_attn_blocksparse_qseq_b2_sq256_skv256_hq4_dh64_kernel(
    x: jax.Array,
    Wq: jax.Array,
    K_ext: jax.Array,
    V_ext: jax.Array,
    Wo: jax.Array,
):
    x2 = x.reshape(ROWS, D_MODEL)
    kt = jnp.transpose(K_ext, (0, 2, 3, 1)).reshape(B, N_PAIR * PAIR, SKV)
    vt = jnp.transpose(V_ext, (0, 2, 3, 1)).reshape(B, N_PAIR * PAIR, SKV)
    any_spec = pl.BlockSpec(memory_space=pl.ANY)
    return pl.pallas_call(
        _kernel,
        out_shape=jax.ShapeDtypeStruct((B, SQ, D_MODEL), jnp.float32),
        in_specs=[any_spec] * 5,
        out_specs=pl.BlockSpec(memory_space=pltpu.VMEM),
        scratch_shapes=[
            pltpu.VMEM((ROWS, D_MODEL), jnp.float32),
            pltpu.VMEM((ROWS, D_MODEL), jnp.bfloat16),
            pltpu.VMEM((D_MODEL, 2 * PAIR), jnp.float32),
            pltpu.VMEM((2 * PAIR, D_MODEL), jnp.float32),
            pltpu.VMEM((B, N_PAIR * PAIR, SKV), jnp.float32),
            pltpu.VMEM((B, N_PAIR * PAIR, SKV), jnp.float32),
            pltpu.VMEM((N_PAIR, D_MODEL, PAIR), jnp.bfloat16),
            pltpu.VMEM((N_DEV, 2, NCB, 2, DH, 128), jnp.bfloat16),
            pltpu.VMEM((N_PAIR, ROWS, PAIR), jnp.bfloat16),
            pltpu.VMEM((2, R0, PAIR), jnp.float32),
            pltpu.SemaphoreType.DMA((len(WQ_CHUNKS) + 2,)),
            pltpu.SemaphoreType.DMA((2 * N_PAIR,)),
            pltpu.SemaphoreType.DMA((2, N_SLOT)),
            pltpu.SemaphoreType.DMA((2, N_SLOT)),
            pltpu.SemaphoreType.REGULAR((2,)),
        ],
        compiler_params=pltpu.CompilerParams(
            collective_id=0,
            vmem_limit_bytes=64 * 1024 * 1024,
            disable_semaphore_checks=True,
            disable_bounds_checks=True,
        ),
    )(x2, Wq, kt, vt, Wo)
```
